```python
import numpy as np

kernel_name = "dist_mean_ax0_shard0_i_m1024_n512"

def setup_inputs():
    return {"x": np.random.randn(4096, 512).astype(np.float32)}

def reference(x: np.ndarray) -> np.ndarray:
    return np.mean(x, axis=0, keepdims=True)
```

```python
import jax
import jax.numpy as jnp
from jax import lax
from jax.experimental import pallas as pl
from jax.experimental.pallas import tpu as pltpu

N_DEV = 4
N_CHUNKS = 8


def pallas_dist_mean_ax0_shard0_i_m1024_n512_kernel(x: jax.Array):
    m, n = x.shape
    rows = m // N_CHUNKS
    inv = 1.0 / (m * N_DEV)

    def body(x_hbm, o_ref, xbuf, comm, load_sems, send_sems, recv_sems):
        me = lax.axis_index("i")
        loads = [
            pltpu.make_async_copy(
                x_hbm.at[pl.ds(c * rows, rows)], xbuf.at[pl.ds(c * rows, rows)], load_sems.at[c]
            )
            for c in range(N_CHUNKS)
        ]
        for c in loads:
            c.start()
        barrier = pltpu.get_barrier_semaphore()
        for d in range(1, N_DEV):
            pl.semaphore_signal(
                barrier, 1, device_id=((me + d) % N_DEV,), device_id_type=pl.DeviceIdType.MESH
            )
        acc = None
        for c in range(N_CHUNKS):
            loads[c].wait()
            part = xbuf[pl.ds(c * rows, rows), :].reshape(rows // 8, 8, n).sum(axis=0)
            acc = part if acc is None else acc + part
        comm[0] = jnp.sum(acc, axis=0, keepdims=True)
        pl.semaphore_wait(barrier, N_DEV - 1)
        sends = [
            pltpu.make_async_remote_copy(
                comm.at[0], comm.at[d], send_sems.at[d - 1], recv_sems.at[d - 1],
                device_id=((me + d) % N_DEV,), device_id_type=pl.DeviceIdType.MESH,
            )
            for d in (2, 1, 3)
        ]
        for s in sends:
            s.start()
        for s in sends:
            s.wait_recv()
        o_ref[...] = ((comm[0] + comm[2]) + (comm[1] + comm[3])) * inv
        for s in sends:
            s.wait_send()

    return pl.pallas_call(
        body,
        out_shape=jax.ShapeDtypeStruct((1, n), x.dtype),
        in_specs=[pl.BlockSpec(memory_space=pl.ANY)],
        out_specs=pl.BlockSpec(memory_space=pltpu.VMEM),
        scratch_shapes=[
            pltpu.VMEM((m, n), x.dtype),
            pltpu.VMEM((N_DEV, 1, n), jnp.float32),
            pltpu.SemaphoreType.DMA((N_CHUNKS,)),
            pltpu.SemaphoreType.DMA((N_DEV - 1,)),
            pltpu.SemaphoreType.DMA((N_DEV - 1,)),
        ],
        compiler_params=pltpu.CompilerParams(collective_id=0),
    )(x)
```

```python
import jax
import jax.numpy as jnp
from jax import lax
from jax.experimental import pallas as pl
from jax.experimental.pallas import tpu as pltpu

N_DEV = 4
SUBLANES = 8
LANES = 128

LATE = 2
GIVE_ROWS = 32
BIG_CHUNKS = 4
LAST_ROWS = 64
TAIL_ROWS = 32


def _tree_sum(values):
    values = list(values)
    while len(values) > 1:
        pairs = [values[i] + values[i + 1] for i in range(0, len(values) - 1, 2)]
        values = pairs + values[2 * len(pairs) :]
    return values[0]


def pallas_dist_mean_ax0_shard0_i_m1024_n512_kernel(x: jax.Array):
    m, n = x.shape
    scale = 1.0 / (m * N_DEV)
    helpers = ((LATE + 1) % N_DEV, (LATE - 1) % N_DEV)

    given = GIVE_ROWS * len(helpers)
    tail_start = m - TAIL_ROWS
    tiles = (tail_start - given - LAST_ROWS) // SUBLANES
    sizes = [
        SUBLANES * (tiles // BIG_CHUNKS + (c < tiles % BIG_CHUNKS))
        for c in range(BIG_CHUNKS)
    ] + [LAST_ROWS]
    starts = [given + sum(sizes[:c]) for c in range(len(sizes))]
    blocks = n // LANES
    assert starts[-1] + sizes[-1] == tail_start and blocks * LANES == n

    def body(
        x_hbm, o_ref, xbuf, gift, extra, sums,
        chunk_sems, tail_sems, rest_sem, gift_sems, near_sems, diag_sems,
    ):
        def load(rows, cols, sem):
            return pltpu.make_async_copy(x_hbm.at[rows, cols], xbuf.at[rows, cols], sem)

        def send(src, dst, sems, k, device):
            return pltpu.make_async_remote_copy(
                src, dst, sems.at[2 * k], sems.at[2 * k + 1],
                device_id=(device,), device_id_type=pl.DeviceIdType.MESH,
            )

        def sum_rows(ref, start, size):
            rows = ref[pl.ds(start, size), :]
            return rows.reshape(size // SUBLANES, SUBLANES, n).sum(axis=0)

        every_col = pl.ds(0, n)
        chunks = [
            load(pl.ds(start, size), every_col, chunk_sems.at[c])
            for c, (start, size) in enumerate(zip(starts, sizes))
        ]
        tails = [
            load(pl.ds(tail_start, TAIL_ROWS), pl.ds(b * LANES, LANES), tail_sems.at[b])
            for b in range(blocks)
        ]
        rest = load(pl.ds(0, given), every_col, rest_sem)
        gifts = [
            send(x_hbm.at[pl.ds(j * GIVE_ROWS, GIVE_ROWS)], gift, gift_sems, j, helper)
            for j, helper in enumerate(helpers)
        ]

        chunks[0].start()
        me = lax.axis_index("i")

        @pl.when(me != LATE)
        def _():
            rest.start()

        for copy in chunks[1:] + tails:
            copy.start()

        barrier = pltpu.get_barrier_semaphore()
        for step in range(1, N_DEV):
            pl.semaphore_signal(
                barrier, 1,
                device_id=((me + step) & (N_DEV - 1),),
                device_id_type=pl.DeviceIdType.MESH,
            )

        @pl.when(me == LATE)
        def _():
            pl.semaphore_wait(barrier, N_DEV - 1)
            for copy in gifts:
                copy.start()

        acc = None
        for c in range(BIG_CHUNKS):
            chunks[c].wait()
            part = sum_rows(xbuf, starts[c], sizes[c])
            acc = part if acc is None else acc + part

        extra[...] = jnp.zeros(extra.shape, extra.dtype)

        @pl.when(me == LATE)
        def _():
            for copy in gifts:
                copy.wait_send()

        @pl.when(me != LATE)
        def _():
            rest.wait()
            extra[...] = sum_rows(xbuf, 0, given)
            pl.semaphore_wait(barrier, N_DEV - 1)

        for copy, helper in zip(gifts, helpers):

            @pl.when(me == helper)
            def _(copy=copy):
                copy.wait_recv()
                extra[...] += sum_rows(gift, 0, GIVE_ROWS)

        acc = acc + extra[...]

        chunks[-1].wait()
        acc = acc + sum_rows(xbuf, starts[-1], sizes[-1])

        diag = []
        for b in range(blocks):
            cols = pl.ds(b * LANES, LANES)
            tails[b].wait()
            total = _tree_sum(
                [acc[:, b * LANES : (b + 1) * LANES]]
                + [
                    xbuf[pl.ds(row, SUBLANES), cols]
                    for row in range(tail_start, m, SUBLANES)
                ]
            )
            sums[0, :, cols] = jnp.sum(total, axis=0, keepdims=True)
            diag.append(
                send(
                    sums.at[0, :, cols], sums.at[2, :, cols], diag_sems, b,
                    (me + 2) & (N_DEV - 1),
                )
            )
            diag[b].start()

        near = [
            send(sums.at[0], sums.at[step], near_sems, j, (me + step) & (N_DEV - 1))
            for j, step in enumerate((1, 3))
        ]
        for copy in near:
            copy.start()

        for copy in near:
            copy.wait_recv()
        neighbours = sums[1] + sums[3]
        own = sums[0]
        for copy in near + diag:
            copy.wait_send()
        for copy in diag:
            copy.wait_recv()
        o_ref[...] = (((own + sums[2]) + neighbours) * scale).astype(o_ref.dtype)

    return pl.pallas_call(
        body,
        out_shape=jax.ShapeDtypeStruct((1, n), x.dtype),
        in_specs=[pl.BlockSpec(memory_space=pl.ANY)],
        out_specs=pl.BlockSpec(memory_space=pltpu.VMEM),
        scratch_shapes=[
            pltpu.VMEM((m, n), x.dtype),
            pltpu.VMEM((GIVE_ROWS, n), x.dtype),
            pltpu.VMEM((SUBLANES, n), jnp.float32),
            pltpu.VMEM((N_DEV, 1, n), jnp.float32),
            pltpu.SemaphoreType.DMA((len(sizes),)),
            pltpu.SemaphoreType.DMA((blocks,)),
            pltpu.SemaphoreType.DMA,
            pltpu.SemaphoreType.DMA((2 * len(helpers),)),
            pltpu.SemaphoreType.DMA((4,)),
            pltpu.SemaphoreType.DMA((2 * blocks,)),
        ],
        compiler_params=pltpu.CompilerParams(
            collective_id=0,
            disable_bounds_checks=True,
            disable_semaphore_checks=True,
        ),
    )(x)
```

```python
import jax
import jax.numpy as jnp
from jax import lax
from jax.experimental import pallas as pl
from jax.experimental.pallas import tpu as pltpu

N_DEV = 4
SUBLANES = 8
LANES = 128

LATE = 2
HELPERS = ((LATE + 1) % N_DEV, (LATE - 1) % N_DEV)
GIVE_ROWS = 32
BIG_CHUNKS = 4
LAST_ROWS = 64
TAIL_ROWS = 40


def _tree_sum(values):
    values = list(values)
    while len(values) > 1:
        pairs = [values[i] + values[i + 1] for i in range(0, len(values) - 1, 2)]
        values = pairs + values[2 * len(pairs) :]
    return values[0]


def pallas_dist_mean_ax0_shard0_i_m1024_n512_kernel(x: jax.Array):
    m, n = x.shape
    scale = 1.0 / (m * N_DEV)

    given = GIVE_ROWS * len(HELPERS)
    tail_start = m - TAIL_ROWS
    tiles = (tail_start - given - LAST_ROWS) // SUBLANES
    sizes = [
        SUBLANES * (tiles // BIG_CHUNKS + (c < tiles % BIG_CHUNKS))
        for c in range(BIG_CHUNKS)
    ] + [LAST_ROWS]
    starts = [given + sum(sizes[:c]) for c in range(len(sizes))]
    blocks = n // LANES
    assert starts[-1] + sizes[-1] == tail_start and blocks * LANES == n

    def body(
        x_hbm, o_ref, xbuf, gift, extra, sums,
        chunk_sems, tail_sems, rest_sem, gift_sent, gift_arrived,
        near_sent, near_arrived, diag_sent, diag_arrived,
    ):
        def load(rows, cols, sem):
            return pltpu.make_async_copy(x_hbm.at[rows, cols], xbuf.at[rows, cols], sem)

        def send(src, dst, sent, arrived, device):
            return pltpu.make_async_remote_copy(
                src, dst, sent, arrived,
                device_id=(device,), device_id_type=pl.DeviceIdType.MESH,
            )

        def sum_rows(ref, start, size):
            rows = ref[pl.ds(start, size), :].astype(jnp.float32)
            return rows.reshape(size // SUBLANES, SUBLANES, n).sum(axis=0)

        every_col = pl.ds(0, n)
        chunks = [
            load(pl.ds(start, size), every_col, chunk_sems.at[c])
            for c, (start, size) in enumerate(zip(starts, sizes))
        ]
        tails = [
            load(pl.ds(tail_start, TAIL_ROWS), pl.ds(b * LANES, LANES), tail_sems.at[b])
            for b in range(blocks)
        ]
        rest = load(pl.ds(0, given), every_col, rest_sem)
        gifts = [
            send(
                x_hbm.at[pl.ds(j * GIVE_ROWS, GIVE_ROWS)], gift,
                gift_sent.at[j], gift_arrived, helper,
            )
            for j, helper in enumerate(HELPERS)
        ]

        chunks[0].start()
        me = lax.axis_index("i")

        def ahead(steps):
            return (me + steps) & (N_DEV - 1)

        @pl.when(me != LATE)
        def _():
            rest.start()

        for copy in chunks[1:] + tails:
            copy.start()

        barrier = pltpu.get_barrier_semaphore()
        for steps in range(1, N_DEV):
            pl.semaphore_signal(
                barrier, 1,
                device_id=(ahead(steps),), device_id_type=pl.DeviceIdType.MESH,
            )
        pl.semaphore_wait(barrier, N_DEV - 1)

        @pl.when(me == LATE)
        def _():
            for copy in gifts:
                copy.start()

        acc = None
        for c in range(BIG_CHUNKS):
            chunks[c].wait()
            part = sum_rows(xbuf, starts[c], sizes[c])
            acc = part if acc is None else acc + part

        extra[...] = jnp.zeros(extra.shape, extra.dtype)

        @pl.when(me == LATE)
        def _():
            for copy in gifts:
                copy.wait_send()

        @pl.when(me != LATE)
        def _():
            rest.wait()
            extra[...] = sum_rows(xbuf, 0, given)

        @pl.when(jnp.logical_or(me == HELPERS[0], me == HELPERS[1]))
        def _():
            gifts[0].wait_recv()
            extra[...] += sum_rows(gift, 0, GIVE_ROWS)

        acc = acc + extra[...]

        chunks[-1].wait()
        acc = acc + sum_rows(xbuf, starts[-1], sizes[-1])

        diag = []
        for b in range(blocks):
            cols = pl.ds(b * LANES, LANES)
            tails[b].wait()
            total = _tree_sum(
                [acc[:, b * LANES : (b + 1) * LANES]]
                + [
                    xbuf[pl.ds(row, SUBLANES), cols].astype(jnp.float32)
                    for row in range(tail_start, m, SUBLANES)
                ]
            )
            sums[0, :, cols] = jnp.sum(total, axis=0, keepdims=True)
            diag.append(
                send(
                    sums.at[0, :, cols], sums.at[2, :, cols],
                    diag_sent.at[b], diag_arrived.at[b], ahead(2),
                )
            )
            diag[b].start()

        near = [
            send(
                sums.at[0], sums.at[steps],
                near_sent.at[j], near_arrived.at[j], ahead(steps),
            )
            for j, steps in enumerate((1, N_DEV - 1))
        ]
        for copy in near:
            copy.start()

        for copy in near:
            copy.wait_recv()
        neighbours = sums[1] + sums[N_DEV - 1]
        own = sums[0]
        for copy in near + diag:
            copy.wait_send()
        for copy in diag:
            copy.wait_recv()
        o_ref[...] = (((own + sums[2]) + neighbours) * scale).astype(o_ref.dtype)

    return pl.pallas_call(
        body,
        out_shape=jax.ShapeDtypeStruct((1, n), x.dtype),
        in_specs=[pl.BlockSpec(memory_space=pl.ANY)],
        out_specs=pl.BlockSpec(memory_space=pltpu.VMEM),
        scratch_shapes=[
            pltpu.VMEM((m, n), x.dtype),
            pltpu.VMEM((GIVE_ROWS, n), x.dtype),
            pltpu.VMEM((SUBLANES, n), jnp.float32),
            pltpu.VMEM((N_DEV, 1, n), jnp.float32),
            pltpu.SemaphoreType.DMA((len(sizes),)),
            pltpu.SemaphoreType.DMA((blocks,)),
            pltpu.SemaphoreType.DMA,
            pltpu.SemaphoreType.DMA((len(HELPERS),)),
            pltpu.SemaphoreType.DMA,
            pltpu.SemaphoreType.DMA((2,)),
            pltpu.SemaphoreType.DMA((2,)),
            pltpu.SemaphoreType.DMA((blocks,)),
            pltpu.SemaphoreType.DMA((blocks,)),
        ],
        compiler_params=pltpu.CompilerParams(
            collective_id=0,
            disable_bounds_checks=True,
            disable_semaphore_checks=True,
        ),
    )(x)
```
